```python
import numpy as np

kernel_name = "dist_max_ax1_xy_m2048_n1024"

def setup_inputs():
    return {"x": np.random.randn(4096, 2048).astype(np.float32)}

def reference(x: np.ndarray) -> np.ndarray:
    return np.max(x, axis=1, keepdims=True)
```

```python
import jax
import jax.numpy as jnp
from jax import lax
from jax.experimental import pallas as pl
from jax.experimental.pallas import tpu as pltpu

LANES = 128
SUB = 8
NEG = -jnp.inf

K_RAW = 104
MID = (384, 384, 384, 384, 256)
TAIL = (96, 24, 8)


def _compiler_params():
    try:
        return pltpu.CompilerParams(collective_id=0, disable_semaphore_checks=True)
    except TypeError:
        return pltpu.CompilerParams(collective_id=0)


def _tree_max(vs):
    while len(vs) > 1:
        nxt = [jnp.maximum(vs[i], vs[i + 1]) for i in range(0, len(vs) - 1, 2)]
        if len(vs) % 2:
            nxt.append(vs[-1])
        vs = nxt
    return vs[0]


def pallas_dist_max_ax1_xy_m2048_n1024_kernel(x: jax.Array):
    m, n = x.shape
    assert sum(MID) == m - 2 * LANES and sum(TAIL) == LANES and n % LANES == 0
    chunks = []
    start = LANES
    for rows in MID + TAIL:
        chunks.append((start, rows))
        start += rows
    n_mid = len(MID)
    bulk = m - LANES

    def body(x_hbm, out_ref, buf, raw, loc, rem, sems, head_sem, send_sems, recv_sems):
        def load(s, r, sem):
            return pltpu.make_async_copy(
                x_hbm.at[pl.ds(s, r), :], buf.at[pl.ds(s, r), :], sem
            )

        loads = [load(s, r, sems.at[i]) for i, (s, r) in enumerate(chunks)]
        loads[0].start()

        my_x = lax.axis_index("x")
        my_y = lax.axis_index("y")
        peer = (my_x, 1 - my_y)
        barrier = pltpu.get_barrier_semaphore()
        pl.semaphore_signal(
            barrier, inc=1, device_id=peer, device_id_type=pl.DeviceIdType.MESH
        )

        def raw_copy():
            return pltpu.make_async_remote_copy(
                src_ref=x_hbm.at[pl.ds(0, K_RAW), :],
                dst_ref=raw,
                send_sem=send_sems.at[2],
                recv_sem=recv_sems.at[2],
                device_id=peer,
                device_id_type=pl.DeviceIdType.MESH,
            )

        def part_copy(lo, size, k):
            return pltpu.make_async_remote_copy(
                src_ref=loc.at[:, pl.ds(lo, size)],
                dst_ref=rem.at[:, pl.ds(lo, size)],
                send_sem=send_sems.at[k],
                recv_sem=recv_sems.at[k],
                device_id=peer,
                device_id_type=pl.DeviceIdType.MESH,
            )

        @pl.when(my_y == 1)
        def _():
            pl.semaphore_wait(barrier, 1)
            raw_copy().start()
            load(K_RAW, LANES - K_RAW, head_sem).start()

        @pl.when(my_y == 0)
        def _():
            load(0, LANES, head_sem).start()

        for c in loads[1:]:
            c.start()

        lane = lax.broadcasted_iota(jnp.int32, (SUB, LANES), 1)
        sub = lax.broadcasted_iota(jnp.int32, (SUB, LANES), 0)
        diag = lane - sub

        def col_max(ref, r0):
            return _tree_max(
                [ref[pl.ds(r0, SUB), pl.ds(c * LANES, LANES)] for c in range(n // LANES)]
            )

        def to_lanes(p, off):
            return jnp.where(diag == off, jnp.max(p, axis=1, keepdims=True), NEG)

        def store_block(b, sels):
            loc[:, pl.ds(b * LANES, LANES)] = jnp.max(
                _tree_max(sels), axis=0, keepdims=True
            )

        for i in range(n_mid):
            s, r = chunks[i]
            loads[i].wait()
            for b in range(s // LANES, (s + r) // LANES):
                store_block(
                    b,
                    [
                        to_lanes(col_max(buf, b * LANES + o), o)
                        for o in range(0, LANES, SUB)
                    ],
                )
            if i == 1:

                @pl.when(my_y == 1)
                def _():
                    load(K_RAW, LANES - K_RAW, head_sem).wait()
                    store_block(
                        0,
                        [to_lanes(col_max(buf, o), o) for o in range(K_RAW, LANES, SUB)],
                    )

        @pl.when(my_y == 0)
        def _():
            load(0, LANES, head_sem).wait()
            raw_copy().wait_recv()
            sels = []
            for o in range(0, LANES, SUB):
                p = col_max(buf, o)
                if o < K_RAW:
                    p = jnp.maximum(p, col_max(raw, o))
                sels.append(to_lanes(p, o))
            store_block(0, sels)
            pl.semaphore_wait(barrier, 1)

        bulk_copy = part_copy(0, bulk, 0)
        bulk_copy.start()

        sels, pending = [], []
        for i in range(n_mid, len(chunks)):
            s, r = chunks[i]
            loads[i].wait()
            pending += [(col_max(buf, o), o - bulk) for o in range(s, s + r, SUB)]
            if i != len(chunks) - 2:
                sels = [_tree_max(sels + [to_lanes(p, o) for p, o in pending])]
                pending = []
        store_block(bulk // LANES, sels)
        tail_copy = part_copy(bulk, LANES, 1)
        tail_copy.start()

        @pl.when(my_y == 1)
        def _():
            raw_copy().wait_send()

        bulk_copy.wait()
        out_ref[:, pl.ds(0, bulk)] = jnp.maximum(
            loc[:, pl.ds(0, bulk)], rem[:, pl.ds(0, bulk)]
        )
        tail_copy.wait()
        out_ref[:, pl.ds(bulk, LANES)] = jnp.maximum(
            loc[:, pl.ds(bulk, LANES)], rem[:, pl.ds(bulk, LANES)]
        )

    out = pl.pallas_call(
        body,
        out_shape=jax.ShapeDtypeStruct((1, m), x.dtype),
        in_specs=[pl.BlockSpec(memory_space=pl.ANY)],
        out_specs=pl.BlockSpec(memory_space=pltpu.VMEM),
        scratch_shapes=[
            pltpu.VMEM((m, n), x.dtype),
            pltpu.VMEM((K_RAW, n), x.dtype),
            pltpu.VMEM((1, m), x.dtype),
            pltpu.VMEM((1, m), x.dtype),
            pltpu.SemaphoreType.DMA((len(chunks),)),
            pltpu.SemaphoreType.DMA,
            pltpu.SemaphoreType.DMA((3,)),
            pltpu.SemaphoreType.DMA((3,)),
        ],
        compiler_params=_compiler_params(),
    )(x)
    return out.reshape(m, 1)
```

```python
import jax
import jax.numpy as jnp
from jax import lax
from jax.experimental import pallas as pl
from jax.experimental.pallas import tpu as pltpu

LANES = 128
SUB = 8
NEG = -jnp.inf


def make(SPLIT=(8, 4, 2), M1_AFTER=1, use_smem=True, bounce_at=1, head_at=3, raw_pos=4, m2_early=False):
  K_RAW = 104
  PHI = 7
  UNIT = 16
  def kern(x):
    m, n = x.shape
    cb = n // LANES
    tiles = m // SUB * cb
    bt = LANES // SUB * cb
    nb = m // LANES
    nr = nb - 1
    nph = bt // UNIT
    s0 = bt - UNIT + PHI
    n_last = 3 * cb
    assert sum(SPLIT) == nr - 1
    xt = x.reshape(m // SUB, SUB, cb, LANES).transpose(0, 2, 1, 3)
    x3 = xt.reshape(tiles, SUB, LANES)
    x4 = xt.reshape(nb, bt, SUB, LANES)

    def body(x3, x4, out_ref, u, head, raw, lastbuf, sbuf, loc, rem, last_src, last_dst,
             ph_sems, misc_sems, send_sems, recv_sems):
        wrap = [
            pltpu.make_async_copy(x3.at[pl.ds(s0 + bt * j, UNIT)], u.at[0, j], ph_sems.at[0])
            for j in range(nr)
        ]

        def phase(h, r0, cnt, sem):
            return pltpu.make_async_copy(
                x4.at[pl.ds(1 + r0, cnt), pl.ds(UNIT * h - UNIT + PHI, UNIT)],
                u.at[h, pl.ds(r0, cnt)], sem)

        phases = [phase(h, 0, nr, ph_sems.at[h]) for h in range(1, nph - 1)]
        fin, r0 = [], 0
        for j, cnt in enumerate(SPLIT):
            fin.append((r0, cnt, phase(nph - 1, r0, cnt, ph_sems.at[nph - 1 + j])))
            r0 += cnt
        l0 = tiles - n_last
        last1 = pltpu.make_async_copy(x3.at[pl.ds(l0, 2 * cb)], lastbuf.at[pl.ds(0, 2 * cb)], ph_sems.at[nph - 1 + len(SPLIT)])
        last2 = pltpu.make_async_copy(x3.at[pl.ds(l0 + 2 * cb, cb)], lastbuf.at[pl.ds(2 * cb, cb)], ph_sems.at[nph + len(SPLIT)])
        odd = pltpu.make_async_copy(x3.at[pl.ds(l0 - 1, 1)], u.at[nph - 1, nr - 1, pl.ds(0, 1)], misc_sems.at[2])
        if use_smem:
            s_in = pltpu.make_async_copy(x3.at[pl.ds(K_RAW, s0 - K_RAW)], sbuf, misc_sems.at[3])
            s_out = pltpu.make_async_copy(sbuf, head.at[pl.ds(K_RAW, s0 - K_RAW)], misc_sems.at[4])
        else:
            s_out = pltpu.make_async_copy(x3.at[pl.ds(K_RAW, s0 - K_RAW)], head.at[pl.ds(K_RAW, s0 - K_RAW)], misc_sems.at[4])

        def head_load():
            return pltpu.make_async_copy(x3.at[pl.ds(0, K_RAW)], head.at[pl.ds(0, K_RAW)], ph_sems.at[nph + 1 + len(SPLIT)])

        for c in wrap[:raw_pos]:
            c.start()
        if use_smem:
            s_in.start()

        my_x = lax.axis_index("x")
        my_y = lax.axis_index("y")
        peer = (my_x, 1 - my_y)
        barrier = pltpu.get_barrier_semaphore()
        pl.semaphore_signal(barrier, inc=1, device_id=peer, device_id_type=pl.DeviceIdType.MESH)

        def remote(src, dst, k):
            return pltpu.make_async_remote_copy(
                src_ref=src, dst_ref=dst, send_sem=send_sems.at[k], recv_sem=recv_sems.at[k],
                device_id=peer, device_id_type=pl.DeviceIdType.MESH)

        def raw_copy():
            return remote(x3.at[pl.ds(0, K_RAW)], raw, 0)

        for c in wrap[raw_pos:]:
            c.start()
        odd.start()
        if not use_smem:
            s_out.start()

        @pl.when(my_y == 0)
        def _():
            head_load().start()

        for c in phases:
            c.start()
        for _, _, c in fin:
            c.start()
        last1.start()
        last2.start()

        @pl.when(my_y == 1)
        def _():
            pl.semaphore_wait(barrier, 1)
            raw_copy().start()

        lane = lax.broadcasted_iota(jnp.int32, (SUB, LANES), 1)
        sub = lax.broadcasted_iota(jnp.int32, (SUB, LANES), 0)
        group = lane // SUB
        on_diag = (lane % SUB) == sub

        def row_max(t):
            return jnp.max(jnp.max(t, axis=-3), axis=-1, keepdims=True)

        def row_max2(t, t1):
            return jnp.max(jnp.maximum(jnp.max(t, axis=-3), t1), axis=-1, keepdims=True)

        def put(acc, g, r):
            return jnp.where(group == g, r, acc)

        def diagonal(acc):
            return jnp.max(jnp.where(on_diag, acc, NEG), axis=-2, keepdims=True)

        for c in wrap:
            c.wait()
        r15 = row_max(u[0, :, pl.ds(1, cb)])
        acc0 = jnp.where(group == 15, r15[0], NEG)
        acc = jnp.broadcast_to(jnp.concatenate([r15[1:], r15[:1]], axis=0), (nr, SUB, LANES))
        for h in range(1, nph - 1):
            phases[h - 1].wait()
            if use_smem and h == bounce_at:
                s_in.wait()
                s_out.start()
            acc = put(acc, 2 * h - 2, row_max2(u[h - 1, :, pl.ds(cb + 1, cb - 1)], u[h, :, 0]))
            acc = put(acc, 2 * h - 1, row_max(u[h, :, pl.ds(1, cb)]))
            if h == head_at:
                s_out.wait()
                acc0 = put(acc0, 13, row_max(head[pl.ds(K_RAW, cb)]))
                acc0 = put(acc0, 14, row_max2(head[pl.ds(K_RAW + cb, cb - 1)], u[0, 0, 0]))
                loc[0] = diagonal(acc0)
        h = nph - 1
        odd.wait()
        mine = diagonal(put(acc[nr - 1], 2 * h - 2, row_max2(u[h - 1, nr - 1, pl.ds(cb + 1, cb - 1)], u[h, nr - 1, 0])))
        loc[nb - 1] = mine

        @pl.when(my_y == 0)
        def _():
            head_load().wait()
            raw_copy().wait_recv()
            g = K_RAW // cb
            t = jnp.maximum(head[pl.ds(0, K_RAW)], raw[...]).reshape(g, cb, SUB, LANES)
            r = row_max(t)
            gi = lax.broadcasted_iota(jnp.int32, (g, SUB, LANES), 0)
            v = jnp.max(jnp.where(group == gi, r, NEG), axis=0)
            loc[0] = jnp.maximum(loc[0], diagonal(v))
            pl.semaphore_wait(barrier, 1)

        for j, (r0, cnt, c) in enumerate(fin):
            c.wait()
            rs = pl.ds(r0, cnt)
            a = acc[r0:r0 + cnt]
            a = put(a, 2 * h - 2, row_max2(u[h - 1, rs, pl.ds(cb + 1, cb - 1)], u[h, rs, 0]))
            a = put(a, 2 * h - 1, row_max(u[h, rs, pl.ds(1, cb)]))
            a = put(a, 2 * h, row_max2(u[h, rs, pl.ds(cb + 1, cb - 1)], u[0, pl.ds(r0 + 1, cnt), 0]))
            if j < len(fin) - 1:
                loc[pl.ds(r0 + 1, cnt)] = diagonal(a)
            if j == M1_AFTER:
                n1 = r0 + cnt + 1
                m1 = remote(loc.at[pl.ds(0, n1)], rem.at[pl.ds(0, n1)], 1)
                m1.start()
        m2 = remote(loc.at[pl.ds(n1, nb - n1)], rem.at[pl.ds(n1, nb - n1)], 2)

        def tree(vs):
            while len(vs) > 1:
                vs = [jnp.maximum(vs[i], vs[i + 1]) for i in range(0, len(vs), 2)]
            return vs[0]

        if m2_early:
            loc[pl.ds(r0 + 1, cnt)] = diagonal(a)
            m2.start()
        last1.wait()
        ps = [tree([lastbuf[k * cb + c] for c in range(cb)]) for k in range(2)]
        if not m2_early:
            loc[pl.ds(r0 + 1, cnt)] = diagonal(a)
            m2.start()
        last2.wait()
        ps.append(tree([lastbuf[2 * cb + c] for c in range(cb)]))
        first = LANES - 3 * SUB
        v = None
        for k, p in enumerate(ps):
            r = jnp.max(p, axis=1, keepdims=True)
            v = jnp.broadcast_to(r, (SUB, LANES)) if v is None else jnp.where(lane >= first + k * SUB, r, v)
        vs = [v] + [pltpu.roll(v, SUB - sh, 0) for sh in range(1, SUB)]
        for sh in (1, 2, 4):
            vs = [jnp.where((lane & sh) != 0, vs[j + 1], vs[j]) for j in range(0, len(vs), 2)]
        last = vs[0][:1]
        last_src[...] = last
        m3 = remote(last_src, last_dst, 3)
        m3.start()

        @pl.when(my_y == 1)
        def _():
            raw_copy().wait_send()

        m1.wait_send()
        m2.wait_send()
        m3.wait_send()
        m1.wait_recv()
        out_ref[pl.ds(0, n1)] = jnp.maximum(loc[pl.ds(0, n1)], rem[pl.ds(0, n1)])
        m2.wait_recv()
        out_ref[pl.ds(n1, nb - 1 - n1)] = jnp.maximum(loc[pl.ds(n1, nb - 1 - n1)], rem[pl.ds(n1, nb - 1 - n1)])
        lane1 = lane[:1]
        res = jnp.where(lane1 >= first, last, jnp.maximum(mine, rem[nb - 1]))
        m3.wait_recv()
        theirs = jnp.full((1, LANES), NEG, x.dtype)
        for j in range(first, LANES):
            theirs = jnp.where(lane1 == j, last_dst[0, j], theirs)
        out_ref[nb - 1] = jnp.maximum(res, theirs)

    out = pl.pallas_call(
        body,
        out_shape=jax.ShapeDtypeStruct((nb, 1, LANES), x.dtype),
        in_specs=[pl.BlockSpec(memory_space=pl.ANY), pl.BlockSpec(memory_space=pl.ANY)],
        out_specs=pl.BlockSpec(memory_space=pltpu.VMEM),
        scratch_shapes=[
            pltpu.VMEM((nph, nr, UNIT, SUB, LANES), x.dtype),
            pltpu.VMEM((s0, SUB, LANES), x.dtype),
            pltpu.VMEM((K_RAW, SUB, LANES), x.dtype),
            pltpu.VMEM((n_last, SUB, LANES), x.dtype),
            pltpu.SMEM((s0 - K_RAW, SUB, LANES), x.dtype),
            pltpu.VMEM((nb, 1, LANES), x.dtype),
            pltpu.VMEM((nb, 1, LANES), x.dtype),
            pltpu.VMEM((1, LANES), x.dtype),
            pltpu.SMEM((1, LANES), x.dtype),
            pltpu.SemaphoreType.DMA((nph + 2 + len(SPLIT),)),
            pltpu.SemaphoreType.DMA((6,)),
            pltpu.SemaphoreType.DMA((4,)),
            pltpu.SemaphoreType.DMA((4,)),
        ],
        compiler_params=pltpu.CompilerParams(collective_id=0, disable_semaphore_checks=True),
    )(x3, x4)
    return out.reshape(m, 1)
  return kern


pallas_dist_max_ax1_xy_m2048_n1024_kernel = make()
```

```python
import jax
import jax.numpy as jnp
from jax import lax
from jax.experimental import pallas as pl
from jax.experimental.pallas import tpu as pltpu

LANES = 128
SUB = 8
NEG = -jnp.inf
UNIT = 16
PHI = 7
K_RAW = 116
SPLIT = (8, 4, 2)
SMEM_IN = (0, 4)
SMEM_OUT = (3, 6)
HEAD_AT = 3


def _compiler_params():
    try:
        return pltpu.CompilerParams(collective_id=0, disable_semaphore_checks=True)
    except TypeError:
        return pltpu.CompilerParams(collective_id=0)


def pallas_dist_max_ax1_xy_m2048_n1024_kernel(x: jax.Array):
    m, n = x.shape
    dt = x.dtype
    cb = n // LANES
    tiles = m // SUB * cb
    bt = LANES // SUB * cb
    nb = m // LANES
    nr = nb - 1
    nph = bt // UNIT
    s0 = bt - UNIT + PHI
    n_last = 2 * UNIT - 1
    nx = len(SMEM_IN)
    n_load_sems = nph + len(SPLIT) + 3
    assert UNIT == 2 * cb and PHI == cb - 1 and sum(SPLIT) == nr - 1 and K_RAW < s0

    def body(x3, x4, out_ref, u, w, head, raw, tail, bounce, loc, rem, last_src,
             last_dst, load_sems, smem_sems, send_sems, recv_sems):
        sems = iter(load_sems.at[i] for i in range(n_load_sems))

        def load(src, dst, sem=None):
            return pltpu.make_async_copy(src, dst, next(sems) if sem is None else sem)

        def units(h, r0, cnt):
            return x4.at[pl.ds(1 + r0, cnt), pl.ds(UNIT * (h - 1) + PHI, UNIT)]

        phases = [load(units(h, 0, nr), u.at[h - 1]) for h in range(2, nph)]
        wrap_sem = next(sems)
        wrap = [
            load(x3.at[pl.ds(s0 + bt * r, k)], w.at[r, pl.ds(0, k)], wrap_sem)
            for r, k in enumerate([UNIT] * (nr - 1) + [1, cb + 1])
        ]
        fin, r0 = [], 0
        for cnt in SPLIT:
            lo, hi = max(r0, nx), r0 + cnt
            fin.append((r0, cnt, load(units(1, lo, hi - lo), u.at[0, pl.ds(lo, hi - lo)])))
            r0 = hi
        t0 = s0 + bt * (nr - 1) + 1
        tail1 = load(x3.at[pl.ds(t0, 3 * cb)], tail.at[pl.ds(0, 3 * cb)])
        tail2 = load(x3.at[pl.ds(t0 + 3 * cb, cb - 1)], tail.at[pl.ds(3 * cb, cb - 1)])
        rest = load(x3.at[pl.ds(K_RAW, s0 - K_RAW)], head.at[pl.ds(K_RAW, s0 - K_RAW)])
        head_sem = next(sems)
        smem_in = [
            load(units(1, j, 1), bounce.at[pl.ds(j, 1)], smem_sems.at[j]) for j in range(nx)
        ]
        smem_out = [load(bounce.at[j], u.at[0, j], smem_sems.at[nx + j]) for j in range(nx)]

        def head_load(dst):
            return load(x3.at[pl.ds(0, K_RAW)], dst, head_sem)

        def smem_step(step):
            for j in range(nx):
                if SMEM_OUT[j] == step:
                    smem_in[j].wait()
                    smem_out[j].start()
            for j in range(nx):
                if SMEM_IN[j] == step:
                    smem_in[j].start()

        phases[0].start()
        smem_step(0)

        my_y = lax.axis_index("y")
        peer = (lax.axis_index("x"), 1 - my_y)
        barrier = pltpu.get_barrier_semaphore()
        pl.semaphore_signal(
            barrier, inc=1, device_id=peer, device_id_type=pl.DeviceIdType.MESH
        )

        def remote(src, dst, k):
            return pltpu.make_async_remote_copy(
                src_ref=src,
                dst_ref=dst,
                send_sem=send_sems.at[k],
                recv_sem=recv_sems.at[k],
                device_id=peer,
                device_id_type=pl.DeviceIdType.MESH,
            )

        def raw_copy():
            return remote(x3.at[pl.ds(0, K_RAW)], raw, 0)

        @pl.when(my_y == 1)
        def _():
            pl.semaphore_wait(barrier, 1)
            raw_copy().start()

        rest.start()

        @pl.when(my_y == 0)
        def _():
            head_load(head.at[pl.ds(0, K_RAW)]).start()

        for c in phases[1:] + wrap + [c for _, _, c in fin] + [tail1, tail2]:
            c.start()

        lane = lax.broadcasted_iota(jnp.int32, (SUB, LANES), 1)
        sub = lax.broadcasted_iota(jnp.int32, (SUB, LANES), 0)
        group = lane // SUB
        on_diag = (lane % SUB) == sub
        odd_tiles, even_tiles = pl.ds(1, cb), pl.ds(cb + 1, cb - 1)

        def row_max(t, t1=None):
            t = jnp.max(t, axis=-3)
            if t1 is not None:
                t = jnp.maximum(t, t1)
            return jnp.max(t, axis=-1, keepdims=True)

        def put(acc, g, r):
            return jnp.where(group == g, r, acc)

        def diagonal(acc):
            return jnp.max(jnp.where(on_diag, acc, NEG), axis=-2, keepdims=True)

        def span_max(ref, lo, hi):
            acc = jnp.full((SUB, LANES), NEG, dt)
            for g in range(lo // cb, -(-hi // cb)):
                a, b = max(lo, g * cb), min(hi, (g + 1) * cb)
                acc = put(acc, g, row_max(ref[pl.ds(a, b - a)]))
            return diagonal(acc)

        acc = None
        for h in range(2, nph):
            phases[h - 2].wait()
            smem_step(h - 1)
            r = row_max(u[h - 1, :, odd_tiles])
            if acc is None:
                acc = jnp.broadcast_to(r, (nr, SUB, LANES))
            else:
                acc = put(acc, 2 * h - 1, r)
                acc = put(acc, 2 * h - 2, row_max(u[h - 2, :, even_tiles], u[h - 1, :, 0]))
            if h - 1 == HEAD_AT:
                rest.wait()
                loc[1] = span_max(head, K_RAW, s0)

                @pl.when(my_y == 0)
                def _():
                    head_load(head.at[pl.ds(0, K_RAW)]).wait()
                    loc[1] = jnp.maximum(loc[1], span_max(head, 0, K_RAW))
                    pl.semaphore_wait(barrier, 1)

        for c in wrap:
            c.wait()
        g_last = 2 * nph - 1
        acc = put(acc, g_last - 1, row_max(u[nph - 2, :, even_tiles], w[pl.ds(1, nr), 0]))
        r = row_max(w[pl.ds(0, nr - 1), odd_tiles])
        r_end = row_max(w[pl.ds(nr, 1), odd_tiles])
        acc = put(acc, g_last, jnp.concatenate([r[1:], r_end, r_end]))
        acc0 = jnp.where(group == g_last, r[0], NEG)
        acc0 = put(acc0, g_last - 1, row_max(w[0, pl.ds(0, 1)]))
        loc[1] = jnp.maximum(loc[1], diagonal(acc0))
        loc[0] = diagonal(acc[nr - 1])
        for c in smem_out:
            c.wait()

        msgs = []
        for r0, cnt, c in fin:
            c.wait()
            rs = pl.ds(r0, cnt)
            a = put(acc[r0 : r0 + cnt], 0, row_max(w[rs, even_tiles], u[0, rs, 0]))
            a = put(a, 1, row_max(u[0, rs, odd_tiles]))
            a = put(a, 2, row_max(u[0, rs, even_tiles], u[1, rs, 0]))
            loc[pl.ds(r0 + 2, cnt)] = diagonal(a)
            lo = r0 + 2 if r0 else 0
            rows = pl.ds(lo, r0 + 2 + cnt - lo)
            c = remote(loc.at[rows], rem.at[rows], 2 + len(msgs))
            c.start()
            msgs.append((r0, cnt, c))

        def col_max(vs):
            while len(vs) > 1:
                vs = [jnp.maximum(vs[i], vs[i + 1]) for i in range(0, len(vs), 2)]
            return vs[0]

        tail1.wait()
        ps = [col_max([tail[g * cb + c] for c in range(cb)]) for g in range(3)]
        end_tile = u[1, nr - 1, 0]
        tail2.wait()
        ps.append(col_max([tail[3 * cb + c] for c in range(cb - 1)] + [end_tile]))
        v = jnp.broadcast_to(jnp.max(ps[0], axis=1, keepdims=True), (SUB, LANES))
        for g in range(3):
            v = put(v, g, jnp.max(ps[g + 1], axis=1, keepdims=True))
        vs = [v] + [pltpu.roll(v, SUB - s, 0) for s in range(1, SUB)]
        for s in (1, 2, 4):
            vs = [jnp.where((lane & s) != 0, vs[j + 1], vs[j]) for j in range(0, len(vs), 2)]
        last = vs[0][:1]
        last_src[...] = last
        last_copy = remote(last_src, last_dst, 1)
        last_copy.start()

        for _, _, c in msgs:
            c.wait_send()

        @pl.when(my_y == 1)
        def _():
            raw_copy().wait_send()
            head_load(raw).start()
            head_load(raw).wait()

        last_copy.wait_send()

        @pl.when(my_y == 0)
        def _():
            raw_copy().wait_recv()

        own0 = jnp.maximum(loc[1], span_max(raw, 0, K_RAW))
        lane1 = lane[:1]
        for r0, cnt, c in msgs:
            c.wait_recv()
            if r0 == 0:
                out_ref[0] = jnp.maximum(own0, rem[1])
                res_b = jnp.where(lane1 < 3 * SUB, last, jnp.maximum(loc[0], rem[0]))
            if r0 + cnt == nr - 1:
                cnt -= 1
                res_a = jnp.where(
                    lane1 >= LANES - SUB, last, jnp.maximum(loc[nb - 1], rem[nb - 1])
                )
            rows = pl.ds(r0 + 2, cnt)
            out_ref[pl.ds(r0 + 1, cnt)] = jnp.maximum(loc[rows], rem[rows])
        last_copy.wait_recv()
        for b, res, lanes in (
            (nb - 2, res_a, range(LANES - SUB, LANES)),
            (nb - 1, res_b, range(3 * SUB)),
        ):
            theirs = jnp.full((1, LANES), NEG, dt)
            for j in lanes:
                theirs = jnp.where(lane1 == j, last_dst[0, j], theirs)
            out_ref[b] = jnp.maximum(res, theirs)

    xt = x.reshape(m // SUB, SUB, cb, LANES).transpose(0, 2, 1, 3)
    out = pl.pallas_call(
        body,
        out_shape=jax.ShapeDtypeStruct((nb, 1, LANES), dt),
        in_specs=[pl.BlockSpec(memory_space=pl.ANY), pl.BlockSpec(memory_space=pl.ANY)],
        out_specs=pl.BlockSpec(memory_space=pltpu.VMEM),
        scratch_shapes=[
            pltpu.VMEM((nph - 1, nr, UNIT, SUB, LANES), dt),
            pltpu.VMEM((nb, UNIT, SUB, LANES), dt),
            pltpu.VMEM((s0, SUB, LANES), dt),
            pltpu.VMEM((K_RAW, SUB, LANES), dt),
            pltpu.VMEM((n_last, SUB, LANES), dt),
            pltpu.SMEM((nx, UNIT, SUB, LANES), dt),
            pltpu.VMEM((nb, 1, LANES), dt),
            pltpu.VMEM((nb, 1, LANES), dt),
            pltpu.VMEM((1, LANES), dt),
            pltpu.SMEM((1, LANES), dt),
            pltpu.SemaphoreType.DMA((n_load_sems,)),
            pltpu.SemaphoreType.DMA((2 * nx,)),
            pltpu.SemaphoreType.DMA((2 + len(SPLIT),)),
            pltpu.SemaphoreType.DMA((2 + len(SPLIT),)),
        ],
        compiler_params=_compiler_params(),
    )(xt.reshape(tiles, SUB, LANES), xt.reshape(nb, bt, SUB, LANES))
    return out.reshape(m, 1)
```
